```python
import numpy as np

kernel_name = "dist_sparse_attn_blocksparse_qseq_b2_sq256_skv256_hq4_dh64"

def setup_inputs():
    x = np.random.randn(2, 1024, 512).astype(np.float32)
    Wq = np.random.randn(512, 1024).astype(np.float32) * 0.02
    K_ext = np.random.randn(2, 256, 16, 64).astype(np.float32)
    V_ext = np.random.randn(2, 256, 16, 64).astype(np.float32)
    Wo = np.random.randn(1024, 512).astype(np.float32) * 0.02
    return {"x": x, "Wq": Wq, "K_ext": K_ext, "V_ext": V_ext, "Wo": Wo}

def reference(x, Wq, K_ext, V_ext, Wo):
    B, Sq, Skv, Hq, Dh = 2, 1024, 256, 16, 64
    Q = (x @ Wq).reshape(B, Sq, Hq, Dh)
    qb = (np.arange(Sq) // 64)[:, None]
    kb = (np.arange(Skv) // 64)[None, :]
    mask = (qb == kb) | (kb == 0) | ((qb + kb) % 3 == 0)
    scores = np.einsum('bihd,bjhd->bhij', Q, K_ext).astype(np.float32) * 0.125
    scores = np.where(mask[None, None, :, :], scores, -1e9)
    scores_max = scores.max(axis=-1, keepdims=True)
    w = np.exp(scores - scores_max)
    row_keep = mask.any(axis=1)
    w_sum = np.where(row_keep[None, None, :, None], w.sum(axis=-1, keepdims=True), 1.0)
    w = w / w_sum
    w = np.where(row_keep[None, None, :, None], w, 0.0)
    ctx = np.einsum('bhij,bjhd->bihd', w, V_ext).reshape(B, Sq, Hq * Dh)
    return ctx @ Wo
```

```python
import jax
import jax.numpy as jnp
import numpy as np
from jax import lax
from jax.experimental import pallas as pl
from jax.experimental.pallas import tpu as pltpu

N_DEV = 4
B = 2
SQ = 256
D_MODEL = 512
BLK = 64
NEG = -1e9
SCALE = 0.125
bf16 = jnp.bfloat16
f32 = jnp.float32
i32 = jnp.int32

PERM = (0, 3, 1, 2)
HEAD = 32
QCH = ((0, HEAD), (32, 32), (64, 64), (128, 128), (256, 256))
NQC = len(QCH)
MESH = pl.DeviceIdType.MESH

UNIT = 104
GRP = 24
DELTA = 8 + 2 * GRP
M_LO = 0x00FF00FF
M_HI = 0x007F007F
M_NIB = 0x0F000F00
M_HB = 0x7F007F00
M_SGN = int(np.int32(np.uint32(0x80008000)))


def _shr(x, n):
    return lax.shift_right_logical(x, jnp.full(x.shape, n, x.dtype)) if n else x


def _shl(x, n):
    return lax.shift_left(x, jnp.full(x.shape, n, x.dtype)) if n else x


def pallas_dist_sparse_attn_blocksparse_qseq_b2_sq256_skv256_hq4_dh64_kernel(
    x: jax.Array,
    Wq: jax.Array,
    K_ext: jax.Array,
    V_ext: jax.Array,
    Wo: jax.Array,
):
    Kt = jnp.transpose(K_ext, (0, 2, 3, 1)).reshape(B, 8, 128, 256)
    Vt = jnp.transpose(V_ext, (0, 2, 3, 1)).reshape(B, 8, 128, 256)

    def body(x_hbm, wq_hbm, k_hbm, v_hbm, wo_hbm, o_ref,
             x32, wq32, wo32, k32, v32, xb, w_all, pk, hdr, wk, wv, ctx, mix, head, raw,
             lsem, ssem, rsem, ready):
        me = lax.axis_index("i")
        left = (me + N_DEV - 1) % N_DEV
        right = (me + 1) % N_DEV
        diag = (me + 2) % N_DEV

        bar = pltpu.get_barrier_semaphore()

        @pl.when(me != 2)
        def _():
            for nbr in (left, right):
                pl.semaphore_signal(bar, inc=1, device_id=(nbr,), device_id_type=MESH)

        ld_wq = [pltpu.make_async_copy(wq_hbm.at[pl.ds(*QCH[i])],
                                       wq32.at[pl.ds(*QCH[i])], lsem.at[i])
                 for i in range(NQC)]
        ld_x = pltpu.make_async_copy(x_hbm, x32, lsem.at[NQC])
        ld_wo = pltpu.make_async_copy(wo_hbm, wo32, lsem.at[NQC + 1])
        gpair = [2 * me, 2 * me + 1, 2 * left + 1, 2 * right,
                 2 * left, 2 * right + 1, 2 * diag, 2 * diag + 1]
        ld_k = [pltpu.make_async_copy(k_hbm.at[:, gpair[i]], k32.at[i],
                                      lsem.at[NQC + 2 + 2 * i]) for i in range(8)]
        ld_v = [pltpu.make_async_copy(v_hbm.at[:, gpair[i]], v32.at[i],
                                      lsem.at[NQC + 3 + 2 * i]) for i in range(8)]

        sends = []
        sem_ids = {}

        def sid(key):
            return sem_ids.setdefault(key, len(sem_ids))

        def rcopy(src, dst, key, dev):
            k = sid(key)
            return pltpu.make_async_remote_copy(
                src_ref=src, dst_ref=dst, send_sem=ssem.at[k],
                recv_sem=rsem.at[k], device_id=(dev,), device_id_type=MESH)

        def send(src, dst, key, dev):
            cp = rcopy(src, dst, key, dev)
            cp.start()
            sends.append(cp)

        def wait_recv(dst, key):
            rcopy(dst, dst, key, me).wait_recv()

        def hdr_row(s):
            return hdr.at[s, pl.ds(0, 1)]

        def pk_rows(s, r0, n):
            return pk.at[s, pl.ds(r0, n)]

        hrows = pl.ds(0, HEAD)

        def head_copy(src, to_right):
            if to_right:
                return rcopy(src.at[hrows, pl.ds(128, 128)], head.at[0], ("hd", 2), right)
            return rcopy(src.at[hrows, pl.ds(0, 128)], head.at[1], ("hd", 3), left)

        @pl.when(me == 1)
        def _():
            pl.semaphore_wait(bar, 1)
            head_copy(wq_hbm, False).start()

        @pl.when(me == 3)
        def _():
            pl.semaphore_wait(bar, 1)
            head_copy(wq_hbm, True).start()

        @pl.when(me == 2)
        def _():
            pl.semaphore_wait(bar, 2)
            head_copy(wq_hbm, True).start()
            head_copy(wq_hbm, False).start()
            for nbr in (left, right):
                pl.semaphore_signal(ready, inc=1, device_id=(nbr,), device_id_type=MESH)

        for i in list(range(1, NQC)) + [0]:
            ld_wq[i].start()
        ld_x.start()
        ld_wo.start()
        for i in range(0, 8):
            ld_k[i].start()
            ld_v[i].start()

        def encode(s):
            w = pltpu.bitcast(w_all[s], i32)
            hi7 = _shr(w, 8) & M_HI
            h_hi = _shr(jnp.max(hi7, axis=0, keepdims=True), 16)
            h_lo = jnp.max(hi7 & 0x7F, axis=0, keepdims=True)
            h = jnp.max(jnp.maximum(h_hi, h_lo), axis=1, keepdims=True)
            h2 = jnp.broadcast_to(h | _shl(h, 16), (1, 128))
            code = h2 - hi7
            over = jnp.max(code & 0x00700070, axis=0, keepdims=True)
            over = jnp.max(over, axis=1, keepdims=True)
            bad = jnp.broadcast_to(jnp.where(over > 0, 1, 0).astype(i32), (1, 128))
            hdr[s, 0:1, :] = _shl(h2, 8) | bad
            for u in range(2):
                r0 = u * UNIT
                sg = None
                for g in range(16):
                    g0 = u * 128 + g * 8
                    t = _shr(w[g0:g0 + 8] & M_SGN, g)
                    sg = t if sg is None else sg | t
                pk[s, r0:r0 + 8, :] = sg
                for k in range(4):
                    g0 = u * 128 + k * 32
                    p0 = r0 + 8 + GRP * k
                    pk[s, p0:p0 + 16, :] = (
                        (w[g0:g0 + 16] & M_LO) | _shl(w[g0 + 16:g0 + 32] & M_LO, 8))
                    nib = None
                    for j in range(4):
                        t = _shl(code[g0 + 8 * j:g0 + 8 * j + 8], 4 * j)
                        nib = t if nib is None else nib | t
                    pk[s, p0 + 16:p0 + 24, :] = nib

        def decode(s, u, ks=(0, 1, 2, 3)):
            r0 = u * UNIT
            hb = hdr[s, 0:1, :] & M_HB
            sg = pk[s, r0:r0 + 8, :]
            for k in ks:
                p0 = r0 + 8 + GRP * k
                lw = pk[s, p0:p0 + 16, :]
                nib = pk[s, p0 + 16:p0 + 24, :]
                nb = jnp.concatenate(
                    [(_shl(nib, 8 - 4 * j) if j <= 2 else _shr(nib, 4)) & M_NIB
                     for j in range(4)], axis=0)
                lo_b = jnp.concatenate([lw & M_LO, _shr(lw, 8) & M_LO], axis=0)
                sgn = jnp.concatenate(
                    [_shl(sg, 4 * k + j) & M_SGN for j in range(4)], axis=0)
                w = lo_b | (hb - nb) | sgn
                rr = u * 256 + k * 64
                w_all[s, rr:rr + 64, :] = pltpu.bitcast(w, bf16)

        to_r = [head_copy(wq32, True)]
        to_l = [head_copy(wq32, False)]
        fast_r = me >= 2
        fast_l = jnp.logical_or(me == 1, me == 2)

        def early(cp, lst, fast):
            lst.append(cp)

            @pl.when(fast)
            def _():
                cp.start()

        for i in list(range(1, NQC)) + [0]:
            ld_wq[i].wait()
            rows = pl.ds(*QCH[i])
            w = wq32[rows, :]
            w_all[0, rows, :] = w[:, 0:128].astype(bf16)
            w_all[1, rows, :] = w[:, 128:256].astype(bf16)
            if 0 < i < NQC - 1:
                early(rcopy(w_all.at[1, rows], w_all.at[2, rows], ("raw", 2, i), right),
                      to_r, fast_r)
                early(rcopy(w_all.at[0, rows], w_all.at[3, rows], ("raw", 3, i), left),
                      to_l, fast_l)
        encode(0)
        encode(1)
        for src, dst, dev, lst, fast in ((1, 2, right, to_r, fast_r),
                                         (0, 3, left, to_l, fast_l)):
            early(rcopy(hdr_row(src), hdr_row(dst), ("h", dst), dev), lst, fast)
            early(rcopy(pk_rows(src, UNIT, UNIT), pk_rows(dst, UNIT, UNIT),
                        ("p", dst), dev), lst, fast)
        for src, dst, dev, lst, fast in ((0, 4, right, to_r, fast_r),
                                         (1, 5, left, to_l, fast_l)):
            early(rcopy(hdr_row(src), hdr_row(dst), ("h", dst), dev), lst, fast)
            early(rcopy(pk.at[src], pk.at[dst], ("p", dst), dev), lst, fast)
        sends.extend(to_r + to_l)

        @pl.when(me == 0)
        def _():
            pl.semaphore_wait(bar, 2)
            for cr, cl in zip(to_r, to_l):
                cr.start()
                cl.start()

        @pl.when(me == 1)
        def _():
            pl.semaphore_wait(ready, 1)
            for cp in to_r:
                cp.start()

        @pl.when(me == 3)
        def _():
            pl.semaphore_wait(ready, 1)
            for cp in to_l:
                cp.start()

        def send_half(src, dst, dev):
            send(hdr_row(src), hdr_row(dst), ("h", dst), dev)
            send(pk.at[src], pk.at[dst], ("p", dst), dev)

        def wait_half(s):
            wait_recv(hdr_row(s), ("h", s))
            wait_recv(pk.at[s], ("p", s))

        lane = lax.broadcasted_iota(jnp.int32, (128, 128), 1)
        row = lax.broadcasted_iota(jnp.int32, (128, 128), 0)
        lo = lane < 64
        top = row < 64
        is0 = me == 0
        slot = [0] + [1 + (3 - kb - me + 6) % 3 for kb in (1, 2, 3)]
        ones_bd = jnp.where(lo == top, 1.0, 0.0).astype(bf16)

        def prep(src, dst, idx, b):
            for j in range(2):
                t = src[idx, b, :, j * 128:(j + 1) * 128]
                tr = pltpu.roll(t, 64, 1)
                we = jnp.where(top, jnp.where(lo, t, 0.0), jnp.where(lo, 0.0, tr))
                wd = jnp.where(top, jnp.where(lo, tr, 0.0), jnp.where(lo, 0.0, t))
                dst[idx, b, slot[2 * j]] = we.astype(bf16)
                dst[idx, b, slot[2 * j + 1]] = wd.astype(bf16)

        def kv_wait(idx):
            ld_k[idx].wait()
            ld_v[idx].wait()

        def prep_nw(idx):
            for b in range(B):
                prep(k32, wk, idx, b)
                prep(v32, wv, idx, b)

        def soft(tiles):
            mx = tiles[0]
            for t in tiles[1:]:
                mx = jnp.maximum(mx, t)
            m1 = jnp.max(jnp.where(lo, mx, -jnp.inf), axis=1, keepdims=True)
            m2 = jnp.max(jnp.where(lo, -jnp.inf, mx), axis=1, keepdims=True)
            m = jnp.where(lo, m1, m2)
            ps = [jnp.exp(t - m) for t in tiles]
            psum = ps[0]
            for p_ in ps[1:]:
                psum = psum + p_
            pm = jnp.concatenate([p_.astype(bf16) for p_ in ps], axis=1)
            return pm, psum.astype(bf16)

        def qproj(idx):
            q = jnp.dot(xb[...], w_all[idx], preferred_element_type=f32)
            return (q * SCALE).astype(bf16)

        def scores(q, idx, b):
            q1 = q[b * SQ: b * SQ + 128]
            q2 = q[b * SQ + 128: b * SQ + 256]
            w = [wk[idx, b, s] for s in range(4)]
            s1 = jnp.dot(q1, jnp.concatenate([w[0], w[1]], axis=1),
                         preferred_element_type=f32)
            s2 = jnp.dot(q2, jnp.concatenate([w[0], w[2], w[3]], axis=1),
                         preferred_element_type=f32)
            p1 = soft([s1[:, 0:128], s1[:, 128:256]])
            tx = jnp.where(jnp.logical_or(top, is0), s2[:, 128:256], NEG)
            ty = jnp.where(jnp.logical_or(jnp.logical_not(top), is0),
                           s2[:, 256:384], NEG)
            p2 = soft([s2[:, 0:128], tx, ty])
            return p1, p2

        def pv(p, idx, b):
            u = [wv[idx, b, s] for s in range(4)]
            for g, (pm, psum) in enumerate(p):
                wm = jnp.concatenate([u[0], u[1]] if g == 0 else [u[0], u[2], u[3]],
                                     axis=1)
                num = lax.dot_general(pm, wm, (((1,), (1,)), ((), ())),
                                      preferred_element_type=f32)
                den = jnp.dot(psum, ones_bd, preferred_element_type=f32)
                r0 = b * SQ + g * 128
                ctx[idx, r0:r0 + 128, :] = (num / den).astype(bf16)

        def attend2(ia, ib, filler=None):
            qa = qproj(ia)
            pa = [scores(qa, ia, b) for b in range(B)]
            qb = qproj(ib)
            if filler is None:
                pb = [scores(qb, ib, b) for b in range(B)]
                for b in range(B):
                    pv(pa[b], ia, b)
            else:
                for b in range(B):
                    pv(pa[b], ia, b)
                pb = [scores(qb, ib, b) for b in range(B)]
                filler()
            for b in range(B):
                pv(pb[b], ib, b)

        def oproj(i0, c, first=False):
            cs = slice(c * 128, (c + 1) * 128)
            w = jnp.concatenate([w_all[8 + i0, cs, :], w_all[9 + i0, cs, :]], axis=0)
            for b in range(B):
                rs = slice(b * SQ, (b + 1) * SQ)
                lhs = jnp.concatenate([ctx[i0, rs, :], ctx[i0 + 1, rs, :]], axis=1)
                o = jnp.dot(lhs, w, preferred_element_type=f32)
                for i, r in enumerate(PERM):
                    piece = o[i * BLK: (i + 1) * BLK]
                    rr = slice(r * BLK, (r + 1) * BLK)
                    if first:
                        o_ref[b, rr, cs] = piece
                    else:
                        o_ref[b, rr, cs] = o_ref[b, rr, cs] + piece

        def oproj_mix(j, c):
            sa, sb = (14, 15) if j == 0 else (15, 14)
            w = jnp.concatenate([w_all[sa, c * 128:c * 128 + 64, :],
                                 w_all[sb, c * 128 + 64:c * 128 + 128, :]], axis=0)
            cs = slice(c * 128, (c + 1) * 128)
            for b in range(B):
                for hh in range(2):
                    r0 = b * SQ + hh * 128
                    o = jnp.dot(mix[j, r0:r0 + 128, :], w, preferred_element_type=f32)
                    for i in range(2):
                        r = PERM[2 * hh + i]
                        rr = slice(r * BLK, (r + 1) * BLK)
                        o_ref[b, rr, cs] = o_ref[b, rr, cs] + o[i * BLK:(i + 1) * BLK]

        def roll_block(qs, i, fill_a, fill_b):
            prep_nw(i)
            prep_nw(i + 1)
            ra = fill_a()
            pa = [scores(qs[0], i, b) for b in range(B)]
            rb = fill_b()
            pb = [scores(qs[1], i + 1, b) for b in range(B)]
            for b in range(B):
                pv(pa[b], i, b)
            for b in range(B):
                pv(pb[b], i + 1, b)
            return [ra, rb]

        def fast_main():
            ld_x.wait()
            for b in range(B):
                for i, r in enumerate(PERM):
                    xb[b * SQ + i * BLK: b * SQ + (i + 1) * BLK, :] = (
                        x32[b, r * BLK:(r + 1) * BLK, :].astype(bf16))
            qs = [qproj(0), qproj(1)]

            ld_wo.wait()
            for h in range(2):
                for c in range(4):
                    w_all[8 + h, c * 128:(c + 1) * 128, :] = (
                        wo32[h * 128:(h + 1) * 128, c * 128:(c + 1) * 128].astype(bf16))
            encode(8)
            encode(9)
            send_half(8, 12, right)
            send_half(9, 13, left)
            for s_, d_, dev in ((9, 10, right), (8, 11, left)):
                send(hdr_row(s_), hdr_row(d_), ("h", d_), dev)
                send(pk_rows(s_, 0, DELTA), pk_rows(d_, 0, DELTA), ("p", d_), dev)

            kv_wait(0)
            kv_wait(1)
            for s in (2, 3):
                wait_recv(head.at[s - 2], ("hd", s))
                for i in range(1, NQC - 1):
                    wait_recv(w_all.at[s, pl.ds(*QCH[i])], ("raw", s, i))
                wait_recv(hdr_row(s), ("h", s))
                wait_recv(pk_rows(s, UNIT, UNIT), ("p", s))
            for s in (2, 3):
                w_all[s, 0:HEAD, :] = head[s - 2].astype(bf16)
                decode(s, 1)
            qs = roll_block(qs, 0, lambda: qproj(2), lambda: qproj(3))

            rest = 2 * UNIT - DELTA
            wait_half(4)
            send_half(4, 6, right)
            send(pk_rows(9, DELTA, rest), pk_rows(10, DELTA, rest), ("p1", 10), right)
            wait_half(5)
            send_half(5, 7, left)
            send(pk_rows(8, DELTA, rest), pk_rows(11, DELTA, rest), ("p1", 11), left)
            kv_wait(2)
            kv_wait(3)
            for s in (4, 5):
                decode(s, 0)
                decode(s, 1)
            qs = roll_block(qs, 2, lambda: qproj(4), lambda: qproj(5))

            def fill0(c0):
                for c in range(c0, c0 + 2):
                    oproj(0, c, first=True)

            kv_wait(4)
            kv_wait(5)
            roll_block(qs, 4, lambda: fill0(0), lambda: fill0(2))

            tiles = ((0, 8 + 2 * GRP), (8 + 2 * GRP, 2 * GRP), (UNIT, 8 + 2 * GRP))

            def fwd_o(src, dst, dev, order):
                send(hdr_row(src), hdr_row(dst), ("h", dst), dev)
                for c, (r, n) in enumerate(tiles):
                    send(pk_rows(src, r, n), pk_rows(dst, r, n), ("t", dst, c), dev)
                for k in order:
                    r = UNIT + 8 + GRP * k
                    send(pk_rows(src, r, GRP), pk_rows(dst, r, GRP), ("l", dst, k), dev)

            wait_half(12)
            fwd_o(12, 14, right, (2, 3))
            wait_half(13)
            fwd_o(13, 15, left, (3, 2))
            kv_wait(6)
            kv_wait(7)
            for s in (10, 11):
                wait_recv(hdr_row(s), ("h", s))
                wait_recv(pk_rows(s, 0, DELTA), ("p", s))
            for s in (12, 13):
                decode(s, 0)
                decode(s, 1)
            for s in (10, 11):
                decode(s, 0, (0, 1))
            for c in range(4):
                oproj(4, c)
            oproj(2, 0)
            prep_nw(6)
            prep_nw(7)

            wait_half(6)
            wait_half(7)
            for s in (6, 7):
                decode(s, 0)
                decode(s, 1)
            attend2(6, 7)
            lo512 = lax.broadcasted_iota(jnp.int32, (B * SQ, 128), 1) < 64
            c6 = ctx[6].astype(f32)
            c7 = ctx[7].astype(f32)
            mix[0] = jnp.where(lo512, c6, c7).astype(bf16)
            mix[1] = jnp.where(lo512, c7, c6).astype(bf16)

            for s in (10, 11):
                wait_recv(pk_rows(s, DELTA, rest), ("p1", s))
            for s in (10, 11):
                decode(s, 0, (2, 3))
                decode(s, 1)
            for c in range(1, 4):
                oproj(2, c)
            for cp in sends[:-12]:
                cp.wait_send()

            for s in (14, 15):
                wait_recv(hdr_row(s), ("h", s))
            for c, (r, n) in enumerate(tiles):
                for s in (14, 15):
                    wait_recv(pk_rows(s, r, n), ("t", s, c))
                if c == 0:
                    flags = hdr[0, 0:1, :]
                    for s in range(1, 16):
                        flags = flags | hdr[s, 0:1, :]
                    any_bad = jnp.max(flags & 1)
                for s in (14, 15):
                    decode(s, c // 2, (0, 1) if c % 2 == 0 else (2, 3))
                oproj(6, c)
            for j in range(2):
                ka = 2 + j
                kb = 3 - j
                wait_recv(pk_rows(14, UNIT + 8 + GRP * ka, GRP), ("l", 14, ka))
                wait_recv(pk_rows(15, UNIT + 8 + GRP * kb, GRP), ("l", 15, kb))
                decode(14, 1, (ka,))
                decode(15, 1, (kb,))
                oproj_mix(j, 3)

            for cp in sends[-12:]:
                cp.wait_send()
            return any_bad

        def fallback():
            plan = ((1, 2, right), (0, 4, right), (0, 3, left), (1, 5, left),
                    (0, 6, diag), (1, 7, diag))
            cps = []
            for base in (0, 8):
                for s_, d_, dev in plan:
                    j = (d_ - 2) + (6 if base else 0)
                    cp = rcopy(w_all.at[base + s_], raw.at[j], ("fb", j), dev)
                    cp.start()
                    cps.append(cp)
            for cp in cps:
                cp.wait()
            for j in range(12):
                w_all[2 + j + (2 if j >= 6 else 0)] = raw[j]
            for c in range(4):
                oproj(0, c, first=True)

            def redo(t, carry):
                i0 = 2 + 2 * t
                attend2(i0, i0 + 1)
                for c in range(4):
                    oproj(i0, c)
                return carry

            lax.fori_loop(0, 3, redo, 0)

        def step(state):
            pl.when(state == 1)(fallback)
            bad = lax.cond(state == 0, fast_main, lambda: jnp.int32(0))
            return jnp.where(bad != 0, 1, 2).astype(jnp.int32)

        lax.while_loop(lambda state: state < 2, step, jnp.int32(0))
        assert len(sem_ids) <= n_rsem, len(sem_ids)

    n_rsem = 54
    return pl.pallas_call(
        body,
        out_shape=jax.ShapeDtypeStruct((B, SQ, D_MODEL), f32),
        in_specs=[pl.BlockSpec(memory_space=pl.ANY)] * 5,
        out_specs=pl.BlockSpec(memory_space=pltpu.VMEM),
        scratch_shapes=[
            pltpu.VMEM((B, SQ, D_MODEL), f32),
            pltpu.VMEM((D_MODEL, 256), f32),
            pltpu.VMEM((256, D_MODEL), f32),
            pltpu.VMEM((8, B, 128, 256), f32),
            pltpu.VMEM((8, B, 128, 256), f32),
            pltpu.VMEM((B * SQ, D_MODEL), bf16),
            pltpu.VMEM((16, 512, 128), bf16),
            pltpu.VMEM((16, 2 * UNIT, 128), i32),
            pltpu.VMEM((16, 8, 128), i32),
            pltpu.VMEM((8, B, 4, 128, 128), bf16),
            pltpu.VMEM((8, B, 4, 128, 128), bf16),
            pltpu.VMEM((8, B * SQ, 128), bf16),
            pltpu.VMEM((2, B * SQ, 128), bf16),
            pltpu.VMEM((2, HEAD, 128), f32),
            pltpu.VMEM((12, 512, 128), bf16),
            pltpu.SemaphoreType.DMA((NQC + 2 + 16,)),
            pltpu.SemaphoreType.DMA((n_rsem,)),
            pltpu.SemaphoreType.DMA((n_rsem,)),
            pltpu.SemaphoreType.REGULAR,
        ],
        compiler_params=pltpu.CompilerParams(
            collective_id=0, vmem_limit_bytes=64 * 1024 * 1024,
            disable_semaphore_checks=True, disable_bounds_checks=True),
    )(x, Wq, Kt, Vt, Wo)
```

```python
import jax
import jax.numpy as jnp
from jax import lax
from jax.experimental import pallas as pl
from jax.experimental.pallas import tpu as pltpu

N_DEV = 4
B = 2
SQ = 256
D_MODEL = 512
BLK = 64
NEG = -1e9
SCALE = 0.125
bf16 = jnp.bfloat16
f32 = jnp.float32
i32 = jnp.int32

PERM = (0, 3, 1, 2)
MESH = pl.DeviceIdType.MESH

HEAD0, HEAD = 256, 32
RAW0, RAWN = HEAD0 + HEAD, 512 - HEAD0 - HEAD
QCH = ((288, 32), (320, 64), (384, 128), (0, 288))
NRAW = 3
NQC = len(QCH)

HDR = 7
P0 = 8
UNIT = 104
GRP = 24
DELTA = 9
NO1 = 2
M_LO = 0x00FF00FF
M_HI = 0x007F007F
M_NIB = 0x0F000F00
M_HB = 0x7F007F00
M_SGN = -0x7FFF8000
SENT_ROWS = 2 * (HEAD + RAWN // 2 + (1 + UNIT) + 5 * (1 + 2 * UNIT))


def _shr(x, n):
    return lax.shift_right_logical(x, jnp.full(x.shape, n, x.dtype)) if n else x


def _shl(x, n):
    return lax.shift_left(x, jnp.full(x.shape, n, x.dtype)) if n else x


def pallas_dist_sparse_attn_blocksparse_qseq_b2_sq256_skv256_hq4_dh64_kernel(
    x: jax.Array,
    Wq: jax.Array,
    K_ext: jax.Array,
    V_ext: jax.Array,
    Wo: jax.Array,
):
    Kt = jnp.transpose(K_ext, (0, 2, 3, 1)).reshape(B, 8, 128, 256)
    Vt = jnp.transpose(V_ext, (0, 2, 3, 1)).reshape(B, 8, 128, 256)

    def body(x_hbm, wq_hbm, k_hbm, v_hbm, wo_hbm, o_ref,
             x32, wq32, wo32, kv32, xb, w_all, pk, wk, wv, ctx, mix, head, raw, tally,
             lsem, ssem, rsem, ready):
        me = lax.axis_index("i")
        left = (me + N_DEV - 1) % N_DEV
        right = (me + 1) % N_DEV
        diag = (me + 2) % N_DEV

        bar = pltpu.get_barrier_semaphore()

        @pl.when(me != 2)
        def _():
            for nbr in (left, right):
                pl.semaphore_signal(bar, inc=1, device_id=(nbr,), device_id_type=MESH)

        sem_ids = {}

        def rcopy(src, dst, key, dev, send_id=0):
            k = sem_ids.setdefault(key, len(sem_ids))
            return pltpu.make_async_remote_copy(
                src_ref=src, dst_ref=dst, send_sem=ssem.at[send_id],
                recv_sem=rsem.at[k], device_id=(dev,), device_id_type=MESH)

        def wait_recv(dst, key):
            rcopy(dst, dst, key, me).wait_recv()

        def pk_rows(s, r0, n):
            return pk.at[s, pl.ds(r0, n)]

        def pk_copy(src, dst, r0, n, key, dev):
            return rcopy(pk_rows(src, r0, n), pk_rows(dst, r0, n), (key, dst), dev)

        def pk_wait(s, r0, n, key):
            wait_recv(pk_rows(s, r0, n), (key, s))

        hrows = pl.ds(HEAD0, HEAD)

        def head_copy(src, to_right):
            if to_right:
                return rcopy(src.at[hrows, pl.ds(128, 128)], head.at[0], ("hd", 2), right)
            return rcopy(src.at[hrows, pl.ds(0, 128)], head.at[1], ("hd", 3), left)

        @pl.when(me == 1)
        def _():
            pl.semaphore_wait(bar, 1)
            head_copy(wq_hbm, False).start()

        @pl.when(me == 3)
        def _():
            pl.semaphore_wait(bar, 1)
            head_copy(wq_hbm, True).start()

        @pl.when(me == 2)
        def _():
            pl.semaphore_wait(bar, 2)
            head_copy(wq_hbm, True).start()
            head_copy(wq_hbm, False).start()
            for nbr in (left, right):
                pl.semaphore_signal(ready, inc=1, device_id=(nbr,), device_id_type=MESH)

        ld_wq = [pltpu.make_async_copy(wq_hbm.at[pl.ds(*QCH[i])],
                                       wq32.at[pl.ds(*QCH[i])], lsem.at[i])
                 for i in range(NQC)]
        ld_x = pltpu.make_async_copy(x_hbm, x32, lsem.at[NQC])
        ld_wo = pltpu.make_async_copy(wo_hbm, wo32, lsem.at[NQC + 1])
        gpair = [2 * me, 2 * me + 1, 2 * left + 1, 2 * right,
                 2 * left, 2 * right + 1, 2 * diag, 2 * diag + 1]
        for cp in ld_wq:
            cp.start()
        ld_x.start()
        ld_wo.start()
        for i in range(8):
            for j, src in enumerate((k_hbm, v_hbm)):
                pltpu.make_async_copy(src.at[:, gpair[i]], kv32.at[i, j],
                                      lsem.at[NQC + 2 + i // 2]).start()

        def kv_wait(i):
            both = kv32.at[pl.ds(i, 2)]
            pltpu.make_async_copy(both, both, lsem.at[NQC + 2 + i // 2]).wait()

        def stats(w):
            hi7 = _shr(w, 8) & M_HI
            lo7 = hi7 & 0x7F
            r = lambda v, f: f(v.reshape(-1, 8, 128), axis=0)
            return (r(hi7, jnp.max), r(lo7, jnp.max), r(hi7, jnp.min), r(lo7, jnp.min))

        def merge(a, b):
            if a is None:
                return b
            return (jnp.maximum(a[0], b[0]), jnp.maximum(a[1], b[1]),
                    jnp.minimum(a[2], b[2]), jnp.minimum(a[3], b[3]))

        def header(s, st):
            mx = jnp.maximum(_shr(st[0], 16), st[1])
            mn = jnp.minimum(_shr(st[2], 16), st[3])
            h = jnp.max(jnp.max(mx, axis=0, keepdims=True), axis=1, keepdims=True)
            m = jnp.min(jnp.min(mn, axis=0, keepdims=True), axis=1, keepdims=True)
            bad = jnp.where(h - m > 15, 1, 0).astype(i32)
            h2 = h | _shl(h, 16)
            pk[s, HDR:HDR + 1, :] = jnp.broadcast_to(_shl(h2, 8) | bad, (1, 128))
            return jnp.broadcast_to(h2, (1, 128))

        def pack(s, u, h2):
            w = pltpu.bitcast(w_all[s, u * 256:(u + 1) * 256, :], i32)
            code = h2 - (_shr(w, 8) & M_HI)
            r0 = P0 + u * UNIT
            sg = None
            for g in range(16):
                t = _shr(w[g * 8:g * 8 + 8] & M_SGN, g)
                sg = t if sg is None else sg | t
            pk[s, r0:r0 + 8, :] = sg
            for k in range(4):
                g0 = k * 32
                p0 = r0 + 8 + GRP * k
                pk[s, p0:p0 + 16, :] = (
                    (w[g0:g0 + 16] & M_LO) | _shl(w[g0 + 16:g0 + 32] & M_LO, 8))
                nib = None
                for j in range(4):
                    t = _shl(code[g0 + 8 * j:g0 + 8 * j + 8], 4 * j)
                    nib = t if nib is None else nib | t
                pk[s, p0 + 16:p0 + 24, :] = nib

        def decode(s, u, ks=(0, 1, 2, 3)):
            r0 = P0 + u * UNIT
            hb = pk[s, HDR:HDR + 1, :] & M_HB
            sg = pk[s, r0:r0 + 8, :]
            for k in ks:
                p0 = r0 + 8 + GRP * k
                lw = pk[s, p0:p0 + 16, :]
                nib = pk[s, p0 + 16:p0 + 24, :]
                nb = jnp.concatenate(
                    [(_shl(nib, 8 - 4 * j) if j <= 2 else _shr(nib, 4)) & M_NIB
                     for j in range(4)], axis=0)
                lo_b = jnp.concatenate([lw & M_LO, _shr(lw, 8) & M_LO], axis=0)
                sgn = jnp.concatenate(
                    [_shl(sg, 4 * k + j) & M_SGN for j in range(4)], axis=0)
                w = lo_b | (hb - nb) | sgn
                rr = u * 256 + k * 64
                w_all[s, rr:rr + 64, :] = pltpu.bitcast(w, bf16)

        def decode_all(s):
            decode(s, 0)
            decode(s, 1)

        to_r = [head_copy(wq32, True)]
        to_l = [head_copy(wq32, False)]
        fast_r = me >= 2
        fast_l = jnp.logical_or(me == 1, me == 2)

        def early(cp, lst, fast):
            lst.append(cp)

            @pl.when(fast)
            def _():
                cp.start()

        st = [None, None]
        for i in range(NQC):
            ld_wq[i].wait()
            rows = pl.ds(*QCH[i])
            w = wq32[rows, :]
            wb = [w[:, 0:128].astype(bf16), w[:, 128:256].astype(bf16)]
            for h in range(2):
                w_all[h, rows, :] = wb[h]
            if i < NRAW:
                early(rcopy(w_all.at[1, rows], w_all.at[2, rows], ("raw", 2), right),
                      to_r, fast_r)
                early(rcopy(w_all.at[0, rows], w_all.at[3, rows], ("raw", 3), left),
                      to_l, fast_l)
            for h in range(2):
                st[h] = merge(st[h], stats(pltpu.bitcast(wb[h], i32)))
        h2 = [header(h, st[h]) for h in range(2)]
        for h in range(2):
            pack(h, 0, h2[h])
        early(pk_copy(1, 2, HDR, 1 + UNIT, "p", right), to_r, fast_r)
        early(pk_copy(0, 3, HDR, 1 + UNIT, "p", left), to_l, fast_l)
        for h in range(2):
            pack(h, 1, h2[h])
        early(pk_copy(0, 4, HDR, 1 + 2 * UNIT, "p", right), to_r, fast_r)
        early(pk_copy(1, 5, HDR, 1 + 2 * UNIT, "p", left), to_l, fast_l)

        @pl.when(me == 0)
        def _():
            pl.semaphore_wait(bar, 2)
            for cr, cl in zip(to_r, to_l):
                cr.start()
                cl.start()

        @pl.when(me == 1)
        def _():
            pl.semaphore_wait(ready, 1)
            for cp in to_r:
                cp.start()

        @pl.when(me == 3)
        def _():
            pl.semaphore_wait(ready, 1)
            for cp in to_l:
                cp.start()

        def send_half(src, dst, dev):
            pk_copy(src, dst, HDR, 1 + 2 * UNIT, "p", dev).start()

        def wait_half(s):
            pk_wait(s, HDR, 1 + 2 * UNIT, "p")

        lane = lax.broadcasted_iota(jnp.int32, (128, 128), 1)
        row = lax.broadcasted_iota(jnp.int32, (128, 128), 0)
        lo = lane < 64
        top = row < 64
        is0 = me == 0
        slot = [0] + [1 + (3 - kb - me + 6) % 3 for kb in (1, 2, 3)]
        ones_bd = jnp.where(lo == top, 1.0, 0.0).astype(bf16)

        def prep(idx):
            for b in range(B):
                for kv, dst in enumerate((wk, wv)):
                    for j in range(2):
                        t = kv32[idx, kv, b, :, j * 128:(j + 1) * 128]
                        tr = pltpu.roll(t, 64, 1)
                        we = jnp.where(top, jnp.where(lo, t, 0.0), jnp.where(lo, 0.0, tr))
                        wd = jnp.where(top, jnp.where(lo, tr, 0.0), jnp.where(lo, 0.0, t))
                        dst[idx, b, slot[2 * j]] = we.astype(bf16)
                        dst[idx, b, slot[2 * j + 1]] = wd.astype(bf16)

        def soft(tiles):
            mx = tiles[0]
            for t in tiles[1:]:
                mx = jnp.maximum(mx, t)
            m1 = jnp.max(jnp.where(lo, mx, -jnp.inf), axis=1, keepdims=True)
            m2 = jnp.max(jnp.where(lo, -jnp.inf, mx), axis=1, keepdims=True)
            m = jnp.where(lo, m1, m2)
            ps = [jnp.exp(t - m) for t in tiles]
            psum = ps[0]
            for p_ in ps[1:]:
                psum = psum + p_
            pm = jnp.concatenate([p_.astype(bf16) for p_ in ps], axis=1)
            return pm, psum.astype(bf16)

        def qproj(idx):
            q = jnp.dot(xb[...], w_all[idx], preferred_element_type=f32)
            return (q * SCALE).astype(bf16)

        def scores(q, idx, b):
            q1 = q[b * SQ: b * SQ + 128]
            q2 = q[b * SQ + 128: b * SQ + 256]
            w = [wk[idx, b, s] for s in range(4)]
            s1 = jnp.dot(q1, jnp.concatenate([w[0], w[1]], axis=1),
                         preferred_element_type=f32)
            s2 = jnp.dot(q2, jnp.concatenate([w[0], w[2], w[3]], axis=1),
                         preferred_element_type=f32)
            p1 = soft([s1[:, 0:128], s1[:, 128:256]])
            tx = jnp.where(jnp.logical_or(top, is0), s2[:, 128:256], NEG)
            ty = jnp.where(jnp.logical_or(jnp.logical_not(top), is0),
                           s2[:, 256:384], NEG)
            p2 = soft([s2[:, 0:128], tx, ty])
            return p1, p2

        def pv(p, idx, b):
            u = [wv[idx, b, s] for s in range(4)]
            for g, (pm, psum) in enumerate(p):
                wm = jnp.concatenate([u[0], u[1]] if g == 0 else [u[0], u[2], u[3]],
                                     axis=1)
                num = lax.dot_general(pm, wm, (((1,), (1,)), ((), ())),
                                      preferred_element_type=f32)
                den = jnp.dot(psum, ones_bd, preferred_element_type=f32)
                r0 = b * SQ + g * 128
                ctx[idx, r0:r0 + 128, :] = (num / den).astype(bf16)

        def attend2(ia, ib):
            qa = qproj(ia)
            pa = [scores(qa, ia, b) for b in range(B)]
            qb = qproj(ib)
            pb = [scores(qb, ib, b) for b in range(B)]
            for b in range(B):
                pv(pa[b], ia, b)
            for b in range(B):
                pv(pb[b], ib, b)

        def roll_block(qs, i, fill_a, fill_b):
            prep(i)
            prep(i + 1)
            ra = fill_a()
            pa = [scores(qs[0], i, b) for b in range(B)]
            rb = fill_b()
            pb = [scores(qs[1], i + 1, b) for b in range(B)]
            for b in range(B):
                pv(pa[b], i, b)
            for b in range(B):
                pv(pb[b], i + 1, b)
            return [ra, rb]

        def oproj(i0, c, first=False):
            cs = slice(c * 128, (c + 1) * 128)
            w = jnp.concatenate([w_all[8 + i0, cs, :], w_all[9 + i0, cs, :]], axis=0)
            for b in range(B):
                rs = slice(b * SQ, (b + 1) * SQ)
                lhs = jnp.concatenate([ctx[i0, rs, :], ctx[i0 + 1, rs, :]], axis=1)
                o = jnp.dot(lhs, w, preferred_element_type=f32)
                for i, r in enumerate(PERM):
                    piece = o[i * BLK: (i + 1) * BLK]
                    rr = slice(r * BLK, (r + 1) * BLK)
                    if first:
                        o_ref[b, rr, cs] = piece
                    else:
                        o_ref[b, rr, cs] = o_ref[b, rr, cs] + piece

        def oproj_mix(j, c):
            sa, sb = (14, 15) if j == 0 else (15, 14)
            w = jnp.concatenate([w_all[sa, c * 128:c * 128 + 64, :],
                                 w_all[sb, c * 128 + 64:c * 128 + 128, :]], axis=0)
            cs = slice(c * 128, (c + 1) * 128)
            for b in range(B):
                for hh in range(2):
                    r0 = b * SQ + hh * 128
                    o = jnp.dot(mix[j, r0:r0 + 128, :], w, preferred_element_type=f32)
                    for i in range(2):
                        r = PERM[2 * hh + i]
                        rr = slice(r * BLK, (r + 1) * BLK)
                        o_ref[b, rr, cs] = o_ref[b, rr, cs] + o[i * BLK:(i + 1) * BLK]

        def fast_main():
            ld_x.wait()
            for b in range(B):
                for i, r in enumerate(PERM):
                    xb[b * SQ + i * BLK: b * SQ + (i + 1) * BLK, :] = (
                        x32[b, r * BLK:(r + 1) * BLK, :].astype(bf16))
            qs = [qproj(0), qproj(1)]

            ld_wo.wait()
            for h in range(2):
                st_o = None
                for c in range(4):
                    wb = wo32[h * 128:(h + 1) * 128, c * 128:(c + 1) * 128].astype(bf16)
                    w_all[8 + h, c * 128:(c + 1) * 128, :] = wb
                    st_o = merge(st_o, stats(pltpu.bitcast(wb, i32)))
                h2o = header(8 + h, st_o)
                pack(8 + h, 0, h2o)
                pack(8 + h, 1, h2o)
            send_half(8, 12, right)
            send_half(9, 13, left)
            pk_copy(9, 10, HDR, DELTA, "p", right).start()
            pk_copy(8, 11, HDR, DELTA, "p", left).start()

            kv_wait(0)
            for s in (2, 3):
                wait_recv(head.at[s - 2], ("hd", s))
                wait_recv(w_all.at[s, pl.ds(RAW0, RAWN)], ("raw", s))
                pk_wait(s, HDR, 1 + UNIT, "p")
            for s in (2, 3):
                w_all[s, HEAD0:HEAD0 + HEAD, :] = head[s - 2].astype(bf16)
                decode(s, 0)
            qs = roll_block(qs, 0, lambda: qproj(2), lambda: qproj(3))

            rest0, rest = HDR + DELTA, 1 + 2 * UNIT - DELTA
            wait_half(4)
            send_half(4, 6, right)
            pk_copy(9, 10, rest0, rest, "p", right).start()
            wait_half(5)
            send_half(5, 7, left)
            pk_copy(8, 11, rest0, rest, "p", left).start()
            kv_wait(2)
            decode_all(4)
            decode_all(5)
            qs = roll_block(qs, 2, lambda: qproj(4), lambda: qproj(5))

            def fill0(c0):
                for c in range(c0, c0 + 2):
                    oproj(0, c, first=True)

            kv_wait(4)
            roll_block(qs, 4, lambda: fill0(0), lambda: fill0(2))

            tiles = ((HDR, 9 + 2 * GRP), (P0 + 8 + 2 * GRP, 2 * GRP),
                     (P0 + UNIT, 8 + 2 * GRP))

            def grp_row(k):
                return P0 + UNIT + 8 + GRP * k

            def fwd_o(src, dst, dev, order):
                for c, (r, n) in enumerate(tiles):
                    pk_copy(src, dst, r, n, ("t", c), dev).start()
                for k in order:
                    pk_copy(src, dst, grp_row(k), GRP, ("l", k), dev).start()

            wait_half(12)
            fwd_o(12, 14, right, (2, 3))
            wait_half(13)
            fwd_o(13, 15, left, (3, 2))
            kv_wait(6)
            decode_all(12)
            decode_all(13)
            for c in range(NO1):
                oproj(4, c)
            prep(6)
            prep(7)

            wait_half(6)
            wait_half(7)
            decode_all(6)
            decode_all(7)
            late = list(range(NO1, 4))
            oproj(4, late.pop(0))
            attend2(6, 7)
            for c in late:
                oproj(4, c)
            lo512 = lax.broadcasted_iota(jnp.int32, (B * SQ, 128), 1) < 64
            c6 = ctx[6].astype(f32)
            c7 = ctx[7].astype(f32)
            mix[0] = jnp.where(lo512, c6, c7).astype(bf16)
            mix[1] = jnp.where(lo512, c7, c6).astype(bf16)

            wait_half(10)
            wait_half(11)
            decode_all(10)
            decode_all(11)
            for c in range(4):
                oproj(2, c)

            for c, (r, n) in enumerate(tiles):
                for s in (14, 15):
                    pk_wait(s, r, n, ("t", c))
                if c == 0:
                    flags = pk[0, HDR:HDR + 1, :]
                    for s in range(1, 16):
                        flags = flags | pk[s, HDR:HDR + 1, :]
                    any_bad = jnp.max(flags & 1)
                for s in (14, 15):
                    decode(s, c // 2, (0, 1) if c % 2 == 0 else (2, 3))
                oproj(6, c)
            for j in range(2):
                ka = 2 + j
                kb = 3 - j
                pk_wait(14, grp_row(ka), GRP, ("l", ka))
                pk_wait(15, grp_row(kb), GRP, ("l", kb))
                decode(14, 1, (ka,))
                decode(15, 1, (kb,))
                oproj_mix(j, 3)

            pltpu.make_async_copy(tally, tally, ssem.at[0]).wait()
            return any_bad

        def fallback():
            plan = ((1, 2, right), (0, 4, right), (0, 3, left), (1, 5, left),
                    (0, 6, diag), (1, 7, diag))
            cps = []
            for base in (0, 8):
                for s_, d_, dev in plan:
                    j = (d_ - 2) + (6 if base else 0)
                    cp = rcopy(w_all.at[base + s_], raw.at[j], ("fb", j), dev, 1)
                    cp.start()
                    cps.append(cp)
            for cp in cps:
                cp.wait()
            for j in range(12):
                w_all[2 + j + (2 if j >= 6 else 0)] = raw[j]
            for c in range(4):
                oproj(0, c, first=True)

            def redo(t, carry):
                i0 = 2 + 2 * t
                attend2(i0, i0 + 1)
                for c in range(4):
                    oproj(i0, c)
                return carry

            lax.fori_loop(0, 3, redo, 0)

        def step(state):
            pl.when(state == 1)(fallback)
            bad = lax.cond(state == 0, fast_main, lambda: jnp.int32(0))
            return jnp.where(bad != 0, 1, 2).astype(jnp.int32)

        lax.while_loop(lambda state: state < 2, step, jnp.int32(0))
        assert len(sem_ids) <= n_rsem, len(sem_ids)

    n_rsem = 36
    return pl.pallas_call(
        body,
        out_shape=jax.ShapeDtypeStruct((B, SQ, D_MODEL), f32),
        in_specs=[pl.BlockSpec(memory_space=pl.ANY)] * 5,
        out_specs=pl.BlockSpec(memory_space=pltpu.VMEM),
        scratch_shapes=[
            pltpu.VMEM((B, SQ, D_MODEL), f32),
            pltpu.VMEM((D_MODEL, 256), f32),
            pltpu.VMEM((256, D_MODEL), f32),
            pltpu.VMEM((8, 2, B, 128, 256), f32),
            pltpu.VMEM((B * SQ, D_MODEL), bf16),
            pltpu.VMEM((16, 512, 128), bf16),
            pltpu.VMEM((16, P0 + 2 * UNIT, 128), i32),
            pltpu.VMEM((8, B, 4, 128, 128), bf16),
            pltpu.VMEM((8, B, 4, 128, 128), bf16),
            pltpu.VMEM((8, B * SQ, 128), bf16),
            pltpu.VMEM((2, B * SQ, 128), bf16),
            pltpu.VMEM((2, HEAD, 128), f32),
            pltpu.VMEM((12, 512, 128), bf16),
            pltpu.VMEM((SENT_ROWS, 128), i32),
            pltpu.SemaphoreType.DMA((NQC + 2 + 4,)),
            pltpu.SemaphoreType.DMA((2,)),
            pltpu.SemaphoreType.DMA((n_rsem,)),
            pltpu.SemaphoreType.REGULAR,
        ],
        compiler_params=pltpu.CompilerParams(
            collective_id=0, vmem_limit_bytes=64 * 1024 * 1024,
            disable_semaphore_checks=True, disable_bounds_checks=True),
    )(x, Wq, Kt, Vt, Wo)
```

```python
import jax
import jax.numpy as jnp
from jax import lax
from jax.experimental import pallas as pl
from jax.experimental.pallas import tpu as pltpu

N_DEV = 4
B = 2
SQ = 256
D_MODEL = 512
BLK = 64
NEG = -1e9
SCALE = 0.125
bf16 = jnp.bfloat16
f32 = jnp.float32
i32 = jnp.int32

PERM = (0, 3, 1, 2)
MESH = pl.DeviceIdType.MESH

HEAD0, HEAD = 448, 32
RAW0, RAWN = HEAD0 + HEAD, 512 - HEAD0 - HEAD
QCH = ((480, 32), (0, 64), (64, 64), (128, 128), (256, 224))
NQC = len(QCH)

H0 = 5
HDR = 7
P0 = 8
GRP = 24
NP = 3 + 8 * GRP
MS0 = 200
NSLOT = 6
DELTA = 3 + 8
NO0 = 2
M_LO = 0x00FF00FF
M_HI = 0x007F007F
M_HB = 0x7F007F00
M_SGN = -0x7FFF8000
FIRST = NP - GRP
SENT_ROWS = 2 * (HEAD + RAWN // 2 + FIRST + 5 * NP)


def _shr(x, n):
    return lax.shift_right_logical(x, jnp.full(x.shape, n, x.dtype)) if n else x


def _shl(x, n):
    return lax.shift_left(x, jnp.full(x.shape, n, x.dtype)) if n else x


def _pk(x):
    return pltpu.bitcast(x, i32)


def _up(x):
    return pltpu.bitcast(x, bf16)


def pallas_dist_sparse_attn_blocksparse_qseq_b2_sq256_skv256_hq4_dh64_kernel(
    x: jax.Array,
    Wq: jax.Array,
    K_ext: jax.Array,
    V_ext: jax.Array,
    Wo: jax.Array,
):
    Kt = jnp.transpose(K_ext, (0, 2, 3, 1)).reshape(B, 8, 128, 256)
    Vt = jnp.transpose(V_ext, (0, 2, 3, 1)).reshape(B, 8, 128, 256)

    def body(x_hbm, wq_hbm, k_hbm, v_hbm, wo_hbm, o_ref,
             x32, wq32, wo32, kv32, xb, w_all, pk, wk, wv, ctx, mix, head, raw, tally,
             lsem, ssem, rsem, ready):
        me = lax.axis_index("i")
        left = (me + N_DEV - 1) % N_DEV
        right = (me + 1) % N_DEV
        diag = (me + 2) % N_DEV

        bar = pltpu.get_barrier_semaphore()

        @pl.when(me != 2)
        def _():
            for nbr in (left, right):
                pl.semaphore_signal(bar, inc=1, device_id=(nbr,), device_id_type=MESH)

        sem_ids = {}

        def rcopy(src, dst, key, dev, send_id=0):
            k = sem_ids.setdefault(key, len(sem_ids))
            return pltpu.make_async_remote_copy(
                src_ref=src, dst_ref=dst, send_sem=ssem.at[send_id],
                recv_sem=rsem.at[k], device_id=(dev,), device_id_type=MESH)

        def wait_recv(dst, key):
            rcopy(dst, dst, key, me).wait_recv()

        def pk_rows(s, r0, n):
            return pk.at[s, pl.ds(r0, n)]

        def pk_copy(src, dst, r0, n, key, dev):
            return rcopy(pk_rows(src, r0, n), pk_rows(dst, r0, n), (key, dst), dev)

        def pk_wait(s, r0, n, key):
            wait_recv(pk_rows(s, r0, n), (key, s))

        hrows = pl.ds(HEAD0, HEAD)

        def head_copy(src, to_right):
            if to_right:
                return rcopy(src.at[hrows, pl.ds(128, 128)], head.at[0], ("hd", 2), right)
            return rcopy(src.at[hrows, pl.ds(0, 128)], head.at[1], ("hd", 3), left)

        @pl.when(me == 1)
        def _():
            pl.semaphore_wait(bar, 1)
            head_copy(wq_hbm, False).start()

        @pl.when(me == 3)
        def _():
            pl.semaphore_wait(bar, 1)
            head_copy(wq_hbm, True).start()

        @pl.when(me == 2)
        def _():
            pl.semaphore_wait(bar, 2)
            head_copy(wq_hbm, True).start()
            head_copy(wq_hbm, False).start()
            for nbr in (left, right):
                pl.semaphore_signal(ready, inc=1, device_id=(nbr,), device_id_type=MESH)

        ld_wq = [pltpu.make_async_copy(wq_hbm.at[pl.ds(*QCH[i])],
                                       wq32.at[pl.ds(*QCH[i])], lsem.at[i])
                 for i in range(NQC)]
        ld_x = pltpu.make_async_copy(x_hbm, x32, lsem.at[NQC])
        ld_wo = pltpu.make_async_copy(wo_hbm, wo32, lsem.at[NQC + 1])
        gpair = [2 * me, 2 * me + 1, 2 * left + 1, 2 * right,
                 2 * left, 2 * right + 1, 2 * diag, 2 * diag + 1]
        for cp in ld_wq:
            cp.start()
        ld_x.start()
        ld_wo.start()
        kv_sem = [NQC + 2 + k for k in (0, 1, 2, 2, 3, 3, 4, 4)]
        for i in range(8):
            for j, src in enumerate((k_hbm, v_hbm)):
                pltpu.make_async_copy(src.at[:, gpair[i]], kv32.at[i, j],
                                      lsem.at[kv_sem[i]]).start()

        def kv_wait(i, n=2):
            both = kv32.at[pl.ds(i, n)]
            pltpu.make_async_copy(both, both, lsem.at[kv_sem[i]]).wait()

        def stats(w):
            hi7 = _shr(w, 8) & M_HI
            lo7 = hi7 & 0x7F
            r = lambda v, f: f(v.reshape(-1, 8, 128), axis=0)
            return (r(hi7, jnp.max), r(lo7, jnp.max), r(hi7, jnp.min), r(lo7, jnp.min))

        def merge(a, b):
            if a is None:
                return b
            return (jnp.maximum(a[0], b[0]), jnp.maximum(a[1], b[1]),
                    jnp.minimum(a[2], b[2]), jnp.minimum(a[3], b[3]))

        def grp_row(g):
            return P0 + GRP * g

        def pack_lo(s, g):
            w = w_all[s, g * 32:(g + 1) * 32, :]
            p0 = grp_row(g)
            pk[s, p0:p0 + 16, :] = (w[0:16] & M_LO) | _shl(w[16:32] & M_LO, 8)

        widx = lax.broadcasted_iota(i32, (16, 128), 0)

        def pack_nib(s, st):
            mx = jnp.maximum(_shr(st[0], 16), st[1])
            mn = jnp.minimum(_shr(st[2], 16), st[3])
            h = jnp.max(jnp.max(mx, axis=0, keepdims=True), axis=1, keepdims=True)
            h2 = jnp.broadcast_to(h | _shl(h, 16), (1, 128))
            wide = jnp.where(h - jnp.min(mn, axis=0, keepdims=True) > 15, 1, 0)
            planes = []
            for u in range(2):
                w = w_all[s, u * 128:(u + 1) * 128, :]
                code = h2 - (_shr(w, 8) & M_HI)
                fld = (code & 0x00070007) | (_shr(w, 12) & 0x00080008)
                top = _shr(code, 3) & 0x00010001
                pl_ = None
                for g in range(16):
                    t = _shl(top[g * 8:g * 8 + 8], g)
                    pl_ = t if pl_ is None else pl_ | t
                planes.append(pl_)
                for k in range(4):
                    p0 = grp_row(4 * u + k)
                    nib = None
                    for j in range(4):
                        g0 = k * 32 + 8 * j
                        t = _shl(fld[g0:g0 + 8], 4 * j)
                        nib = t if nib is None else nib | t
                    pk[s, p0 + 16:p0 + 24, :] = nib
            return jnp.concatenate(planes, axis=0), _shl(h2, 8) | wide

        def pack_hdr(s, m, hd):
            rows = [None, None]
            for j in range(NSLOT):
                low = m & (0 - m)
                key = jnp.where(m != 0, widx * 32 + (31 - lax.clz(low)), 1023)
                kmin = jnp.min(key, axis=0, keepdims=True)
                m = jnp.where(key == kmin, m ^ low, m)
                t = _shl(kmin, 10 * (j % 3))
                rows[j // 3] = t if rows[j // 3] is None else rows[j // 3] | t
            left_over = jnp.max(jnp.where(m != 0, 1, 0), axis=0, keepdims=True)
            pk[s, H0:H0 + 1, :] = rows[0]
            pk[s, H0 + 1:H0 + 2, :] = rows[1]
            pk[s, HDR:HDR + 1, :] = hd | left_over

        def expand(s):
            m = jnp.zeros((16, 128), i32)
            for j in range(NSLOT):
                r = pk[s, H0 + j // 3:H0 + j // 3 + 1, :]
                f = _shr(r, 10 * (j % 3)) & 1023
                bit = lax.shift_left(jnp.ones((1, 128), i32), f & 31)
                m = m | jnp.where(widx == _shr(f, 5), bit, 0)
            pk[s, MS0:MS0 + 16, :] = m

        def decode(s, gs):
            hb = pk[s, HDR:HDR + 1, :] & M_HB
            for g in gs:
                u, k = g // 4, g % 4
                ms = pk[s, MS0 + 8 * u:MS0 + 8 * u + 8, :]
                p0 = grp_row(g)
                lw = pk[s, p0:p0 + 16, :]
                nib = pk[s, p0 + 16:p0 + 24, :]
                parts = []
                for j in range(4):
                    c3 = (_shl(nib, 8 - 4 * j) if j <= 2 else _shr(nib, 4)) & 0x07000700
                    g16 = 4 * k + j
                    t8 = (_shl(ms, 11 - g16) if g16 <= 11 else _shr(ms, g16 - 11))
                    sgn = _shl(nib, 12 - 4 * j) & M_SGN
                    parts.append((hb - (c3 | (t8 & 0x08000800))) | sgn)
                lo_b = jnp.concatenate([lw & M_LO, _shr(lw, 8) & M_LO], axis=0)
                w = lo_b | jnp.concatenate(parts, axis=0)
                w_all[s, g * 32:(g + 1) * 32, :] = w

        def decode_all(s):
            expand(s)
            decode(s, range(8))

        to_r = [head_copy(wq32, True)]
        to_l = [head_copy(wq32, False)]
        fast_r = me >= 2
        fast_l = jnp.logical_or(me == 1, me == 2)

        def early(cp, lst, fast):
            lst.append(cp)

            @pl.when(fast)
            def _():
                cp.start()

        def early_pk(r0, n):
            early(pk_copy(1, 2, r0, n, "p", right), to_r, fast_r)
            early(pk_copy(0, 3, r0, n, "p", left), to_l, fast_l)

        st = [None, None]
        for i, (r0, n) in enumerate(QCH):
            ld_wq[i].wait()
            rows = pl.ds(r0, n)
            w = wq32[rows, :]
            wb = [_pk(w[:, 0:128].astype(bf16)), _pk(w[:, 128:256].astype(bf16))]
            rows = pl.ds(r0 // 2, n // 2)
            for h in range(2):
                w_all[h, rows, :] = wb[h]
            if i == 0:
                early(rcopy(w_all.at[1, rows], w_all.at[2, rows], ("raw", 2), right),
                      to_r, fast_r)
                early(rcopy(w_all.at[0, rows], w_all.at[3, rows], ("raw", 3), left),
                      to_l, fast_l)
            else:
                gs = range(r0 // 64, (r0 + n) // 64)
                for g in gs:
                    for h in range(2):
                        pack_lo(h, g)
                for g in gs:
                    early_pk(grp_row(g), 16)
            for h in range(2):
                st[h] = merge(st[h], stats(wb[h]))
        mh = [pack_nib(h, st[h]) for h in range(2)]
        for g in range(7):
            early_pk(grp_row(g) + 16, 8)
        for h in range(2):
            pack_lo(h, 7)
            pack_hdr(h, *mh[h])
        early_pk(H0, 3)
        early(pk_copy(0, 4, H0, NP, "p", right), to_r, fast_r)
        early(pk_copy(1, 5, H0, NP, "p", left), to_l, fast_l)

        @pl.when(me == 0)
        def _():
            pl.semaphore_wait(bar, 2)
            for cr, cl in zip(to_r, to_l):
                cr.start()
                cl.start()

        @pl.when(me == 1)
        def _():
            pl.semaphore_wait(ready, 1)
            for cp in to_r:
                cp.start()

        @pl.when(me == 3)
        def _():
            pl.semaphore_wait(ready, 1)
            for cp in to_l:
                cp.start()

        def send_half(src, dst, dev):
            pk_copy(src, dst, H0, NP, "p", dev).start()

        def wait_half(s):
            pk_wait(s, H0, NP, "p")

        lane = lax.broadcasted_iota(jnp.int32, (128, 128), 1)
        row = lax.broadcasted_iota(jnp.int32, (128, 128), 0)
        lo = lane < 64
        top = row < 64
        is0 = me == 0
        slot = [0] + [1 + (3 - kb - me + 6) % 3 for kb in (1, 2, 3)]
        ones_bd = jnp.where(lo == top, 1.0, 0.0).astype(bf16)

        def prep(idx):
            for b in range(B):
                for kv, dst in enumerate((wk, wv)):
                    for j in range(2):
                        t = kv32[idx, kv, b, :, j * 128:(j + 1) * 128]
                        tr = pltpu.roll(t, 64, 1)
                        we = jnp.where(top, jnp.where(lo, t, 0.0), jnp.where(lo, 0.0, tr))
                        wd = jnp.where(top, jnp.where(lo, tr, 0.0), jnp.where(lo, 0.0, t))
                        dst[idx, b, slot[2 * j]] = _pk(we.astype(bf16))
                        dst[idx, b, slot[2 * j + 1]] = _pk(wd.astype(bf16))

        def soft(tiles):
            mx = tiles[0]
            for t in tiles[1:]:
                mx = jnp.maximum(mx, t)
            m1 = jnp.max(jnp.where(lo, mx, -jnp.inf), axis=1, keepdims=True)
            m2 = jnp.max(jnp.where(lo, -jnp.inf, mx), axis=1, keepdims=True)
            m = jnp.where(lo, m1, m2)
            ps = [jnp.exp(t - m) for t in tiles]
            psum = ps[0]
            for p_ in ps[1:]:
                psum = psum + p_
            pm = jnp.concatenate([p_.astype(bf16) for p_ in ps], axis=1)
            return pm, psum.astype(bf16)

        def qproj(idx):
            q = jnp.dot(_up(xb[...]), _up(w_all[idx]), preferred_element_type=f32)
            return (q * SCALE).astype(bf16)

        def scores(q, idx, b):
            q1 = q[b * SQ: b * SQ + 128]
            q2 = q[b * SQ + 128: b * SQ + 256]
            w = [_up(wk[idx, b, s]) for s in range(4)]
            s1 = jnp.dot(q1, jnp.concatenate([w[0], w[1]], axis=1),
                         preferred_element_type=f32)
            s2 = jnp.dot(q2, jnp.concatenate([w[0], w[2], w[3]], axis=1),
                         preferred_element_type=f32)
            p1 = soft([s1[:, 0:128], s1[:, 128:256]])
            tx = jnp.where(jnp.logical_or(top, is0), s2[:, 128:256], NEG)
            ty = jnp.where(jnp.logical_or(jnp.logical_not(top), is0),
                           s2[:, 256:384], NEG)
            p2 = soft([s2[:, 0:128], tx, ty])
            return p1, p2

        def pv(p, idx, b):
            u = [_up(wv[idx, b, s]) for s in range(4)]
            for g, (pm, psum) in enumerate(p):
                wm = jnp.concatenate([u[0], u[1]] if g == 0 else [u[0], u[2], u[3]],
                                     axis=1)
                num = lax.dot_general(pm, wm, (((1,), (1,)), ((), ())),
                                      preferred_element_type=f32)
                den = jnp.dot(psum, ones_bd, preferred_element_type=f32)
                r0 = b * SQ + g * 128
                ctx[idx, r0 // 2:r0 // 2 + 64, :] = _pk((num / den).astype(bf16))

        def attend2(ia, ib):
            qa = qproj(ia)
            pa = [scores(qa, ia, b) for b in range(B)]
            qb = qproj(ib)
            pb = [scores(qb, ib, b) for b in range(B)]
            for b in range(B):
                pv(pa[b], ia, b)
            for b in range(B):
                pv(pb[b], ib, b)

        def roll_block(qs, i, fill_a, fill_b):
            prep(i)
            prep(i + 1)
            ra = fill_a()
            pa = [scores(qs[0], i, b) for b in range(B)]
            rb = fill_b()
            pb = [scores(qs[1], i + 1, b) for b in range(B)]
            for b in range(B):
                pv(pa[b], i, b)
            for b in range(B):
                pv(pb[b], i + 1, b)
            return [ra, rb]

        def oproj(i0, c, first=False):
            cs = slice(c * 128, (c + 1) * 128)
            ws = slice(c * 64, (c + 1) * 64)
            w = _up(jnp.concatenate([w_all[8 + i0, ws, :], w_all[9 + i0, ws, :]], axis=0))
            for b in range(B):
                rs = slice(b * SQ // 2, (b + 1) * SQ // 2)
                lhs = _up(jnp.concatenate([ctx[i0, rs, :], ctx[i0 + 1, rs, :]], axis=1))
                o = jnp.dot(lhs, w, preferred_element_type=f32)
                for i, r in enumerate(PERM):
                    piece = o[i * BLK: (i + 1) * BLK]
                    rr = slice(r * BLK, (r + 1) * BLK)
                    if first:
                        o_ref[b, rr, cs] = piece
                    else:
                        o_ref[b, rr, cs] = o_ref[b, rr, cs] + piece

        def oproj_mix(j, c):
            sa, sb = (14, 15) if j == 0 else (15, 14)
            w = _up(jnp.concatenate([w_all[sa, c * 64:c * 64 + 32, :],
                                     w_all[sb, c * 64 + 32:c * 64 + 64, :]], axis=0))
            cs = slice(c * 128, (c + 1) * 128)
            for b in range(B):
                for hh in range(2):
                    r0 = b * SQ + hh * 128
                    o = jnp.dot(_up(mix[j, r0 // 2:r0 // 2 + 64, :]), w,
                                preferred_element_type=f32)
                    for i in range(2):
                        r = PERM[2 * hh + i]
                        rr = slice(r * BLK, (r + 1) * BLK)
                        o_ref[b, rr, cs] = o_ref[b, rr, cs] + o[i * BLK:(i + 1) * BLK]

        def fast_main():
            ld_x.wait()
            for b in range(B):
                for i, r in enumerate(PERM):
                    x0 = (b * SQ + i * BLK) // 2
                    xb[x0:x0 + BLK // 2, :] = _pk(
                        x32[b, r * BLK:(r + 1) * BLK, :].astype(bf16))
            qs = [qproj(0), qproj(1)]

            ld_wo.wait()
            for h in range(2):
                st_o = None
                for c in range(4):
                    wb = _pk(wo32[h * 128:(h + 1) * 128, c * 128:(c + 1) * 128].astype(bf16))
                    w_all[8 + h, c * 64:(c + 1) * 64, :] = wb
                    st_o = merge(st_o, stats(wb))
                for g in range(8):
                    pack_lo(8 + h, g)
                pack_hdr(8 + h, *pack_nib(8 + h, st_o))
            send_half(9, 10, right)
            send_half(8, 11, left)
            pk_copy(8, 12, H0, DELTA, "p", right).start()
            pk_copy(9, 13, H0, DELTA, "p", left).start()

            kv_wait(0, 1)
            prep(0)
            p0_ = [scores(qs[0], 0, b) for b in range(B)]
            for b in range(B):
                pv(p0_[b], 0, b)

            def own_tiles(cs):
                for c in cs:
                    oproj(0, c, first=True)

            kv_wait(1, 1)
            for s in (2, 3):
                wait_recv(head.at[s - 2], ("hd", s))
                wait_recv(w_all.at[s, pl.ds(RAW0 // 2, RAWN // 2)], ("raw", s))
                pk_wait(s, H0, FIRST, "p")
            for s in (2, 3):
                w_all[s, HEAD0 // 2:(HEAD0 + HEAD) // 2, :] = _pk(head[s - 2].astype(bf16))
                expand(s)
                decode(s, range(7))
            prep(1)
            q2 = qproj(2)
            p1_ = [scores(qs[1], 1, b) for b in range(B)]
            q3 = qproj(3)
            for b in range(B):
                pv(p1_[b], 1, b)
            own_tiles(range(NO0))
            qs = [q2, q3]

            rest0, rest = H0 + DELTA, NP - DELTA
            wait_half(4)
            send_half(4, 6, right)
            pk_copy(8, 12, rest0, rest, "p", right).start()
            wait_half(5)
            send_half(5, 7, left)
            pk_copy(9, 13, rest0, rest, "p", left).start()
            kv_wait(2)
            decode_all(4)
            decode_all(5)
            qs = roll_block(qs, 2, lambda: qproj(4), lambda: qproj(5))

            tiles = ((H0, 3 + 2 * GRP), (grp_row(2), 2 * GRP), (grp_row(4), 2 * GRP))

            def fwd_o(src, dst, dev, order):
                for c, (r, n) in enumerate(tiles):
                    pk_copy(src, dst, r, n, ("t", c), dev).start()
                for k in order:
                    pk_copy(src, dst, grp_row(4 + k), GRP, ("l", k), dev).start()

            wait_half(10)
            fwd_o(10, 15, right, (3, 2))
            wait_half(11)
            fwd_o(11, 14, left, (2, 3))
            kv_wait(4)
            decode_all(10)
            decode_all(11)

            def nbr_tiles(cs):
                for c in cs:
                    oproj(2, c)

            roll_block(qs, 4, lambda: own_tiles(range(NO0, 4)),
                       lambda: nbr_tiles(range(NO0)))

            kv_wait(6)
            nbr_tiles(range(NO0, 4))
            prep(6)
            prep(7)

            wait_half(6)
            wait_half(7)
            decode_all(6)
            decode_all(7)
            attend2(6, 7)
            lo512 = lax.broadcasted_iota(jnp.int32, (B * SQ // 2, 128), 1) < 64
            c6 = ctx[6]
            c7 = ctx[7]
            mix[0] = jnp.where(lo512, c6, c7)
            mix[1] = jnp.where(lo512, c7, c6)

            wait_half(12)
            wait_half(13)
            decode_all(12)
            decode_all(13)
            for c in range(4):
                oproj(4, c)

            for c, (r, n) in enumerate(tiles):
                for s in (14, 15):
                    pk_wait(s, r, n, ("t", c))
                if c == 0:
                    flags = pk[0, HDR:HDR + 1, :]
                    for s in range(1, 16):
                        flags = flags | pk[s, HDR:HDR + 1, :]
                    any_bad = jnp.max(flags & 1)
                for s in (14, 15):
                    if c == 0:
                        expand(s)
                    decode(s, (2 * c, 2 * c + 1))
                oproj(6, c)
            for j in range(2):
                ka = 2 + j
                kb = 3 - j
                pk_wait(14, grp_row(4 + ka), GRP, ("l", ka))
                pk_wait(15, grp_row(4 + kb), GRP, ("l", kb))
                decode(14, (4 + ka,))
                decode(15, (4 + kb,))
                oproj_mix(j, 3)

            pltpu.make_async_copy(tally, tally, ssem.at[0]).wait()
            return any_bad

        def fallback():
            plan = ((1, 2, right), (0, 4, right), (0, 3, left), (1, 5, left),
                    (0, 6, diag), (1, 7, diag))
            cps = []
            for base in (0, 8):
                for s_, d_, dev in plan:
                    j = (d_ - 2) + (6 if base else 0)
                    cp = rcopy(w_all.at[base + s_], raw.at[j], ("fb", j), dev, 1)
                    cp.start()
                    cps.append(cp)
            for cp in cps:
                cp.wait()
            for j in range(12):
                w_all[2 + j + (2 if j >= 6 else 0)] = raw[j]
            for c in range(4):
                oproj(0, c, first=True)

            def redo(t, carry):
                i0 = 2 + 2 * t
                attend2(i0, i0 + 1)
                for c in range(4):
                    oproj(i0, c)
                return carry

            lax.fori_loop(0, 3, redo, 0)

        def step(state):
            pl.when(state == 1)(fallback)
            bad = lax.cond(state == 0, fast_main, lambda: jnp.int32(0))
            return jnp.where(bad != 0, 1, 2).astype(jnp.int32)

        lax.while_loop(lambda state: state < 2, step, jnp.int32(0))
        assert len(sem_ids) <= n_rsem, len(sem_ids)

    n_rsem = 36
    return pl.pallas_call(
        body,
        out_shape=jax.ShapeDtypeStruct((B, SQ, D_MODEL), f32),
        in_specs=[pl.BlockSpec(memory_space=pl.ANY)] * 5,
        out_specs=pl.BlockSpec(memory_space=pltpu.VMEM),
        scratch_shapes=[
            pltpu.VMEM((B, SQ, D_MODEL), f32),
            pltpu.VMEM((D_MODEL, 256), f32),
            pltpu.VMEM((256, D_MODEL), f32),
            pltpu.VMEM((8, 2, B, 128, 256), f32),
            pltpu.VMEM((B * SQ // 2, D_MODEL), i32),
            pltpu.VMEM((16, 256, 128), i32),
            pltpu.VMEM((16, MS0 + 16, 128), i32),
            pltpu.VMEM((8, B, 4, 64, 128), i32),
            pltpu.VMEM((8, B, 4, 64, 128), i32),
            pltpu.VMEM((8, B * SQ // 2, 128), i32),
            pltpu.VMEM((2, B * SQ // 2, 128), i32),
            pltpu.VMEM((2, HEAD, 128), f32),
            pltpu.VMEM((12, 256, 128), i32),
            pltpu.VMEM((SENT_ROWS, 128), i32),
            pltpu.SemaphoreType.DMA((NQC + 2 + 5,)),
            pltpu.SemaphoreType.DMA((2,)),
            pltpu.SemaphoreType.DMA((n_rsem,)),
            pltpu.SemaphoreType.REGULAR,
        ],
        compiler_params=pltpu.CompilerParams(
            collective_id=0, vmem_limit_bytes=64 * 1024 * 1024,
            disable_semaphore_checks=True, disable_bounds_checks=True),
    )(x, Wq, Kt, Vt, Wo)
```
